```python
import numpy as np

kernel_name = "dist_sparse_attn_strided_htp_bs_b2_sq256_skv256_hq4_dh64"

def setup_inputs():
    x = np.random.randn(8, 256, 512).astype(np.float32)
    Wq = np.random.randn(512, 1024).astype(np.float32) * 0.02
    K_ext = np.random.randn(8, 256, 16, 64).astype(np.float32)
    V_ext = np.random.randn(8, 256, 16, 64).astype(np.float32)
    Wo = np.random.randn(1024, 512).astype(np.float32) * 0.02
    return {"x": x, "Wq": Wq, "K_ext": K_ext, "V_ext": V_ext, "Wo": Wo}

def reference(x, Wq, K_ext, V_ext, Wo):
    B, Sq, Skv, Hq, Dh = 8, 256, 256, 16, 64
    Q = (x @ Wq).reshape(B, Sq, Hq, Dh)
    qb = (np.arange(Sq) // 64)[:, None]
    kb = (np.arange(Skv) // 64)[None, :]
    mask = (qb == kb) | ((kb % 4) == (qb % 4))
    scores = np.einsum('bihd,bjhd->bhij', Q, K_ext).astype(np.float32) * 0.125
    scores = np.where(mask[None, None, :, :], scores, -1e9)
    scores_max = scores.max(axis=-1, keepdims=True)
    w = np.exp(scores - scores_max)
    row_keep = mask.any(axis=1)
    w_sum = np.where(row_keep[None, None, :, None], w.sum(axis=-1, keepdims=True), 1.0)
    w = w / w_sum
    w = np.where(row_keep[None, None, :, None], w, 0.0)
    ctx = np.einsum('bhij,bjhd->bihd', w, V_ext).reshape(B, Sq, Hq * Dh)
    return ctx @ Wo
```

```python
import contextlib
import functools

import jax
import jax.numpy as jnp
from jax import lax
from jax.experimental import pallas as pl
from jax.experimental.pallas import tpu as pltpu

N_DEV = 4
B_LOC = 2
SEQ = 256
D_MODEL = 512
TOK = B_LOC * SEQ
DH = 64
BLK = 64
GRP = 256
PAIR = 128
SCALE = 0.125 * 1.4426950408889634

OWN, LEFT, RIGHT, DIAG = range(4)
MESH = pl.DeviceIdType.MESH
BF16 = jnp.bfloat16
F32 = jnp.float32
U32 = jnp.uint32


def to_words(v):
    return pltpu.bitcast(v.astype(BF16), U32)


def from_words(w):
    return pltpu.bitcast(w, BF16)


def make(out_dtype=BF16, scopes=False, asym=True, first_rows=128, nochk=True, qsplit=False):
    def scope(name):
        return jax.named_scope(name) if scopes else contextlib.nullcontext()

    def body(x_hbm, wq_hbm, kt_hbm, vt_hbm, wo_hbm, out_ref,
             x_f32, wq_f32, wo_f32, k_f32, v_f32,
             x_bf, wq_all, wo_all, k_lhs, ctx, acc,
             ld_sem, send_sem, recv_sem, ready_sem):
        me = lax.axis_index("i")
        left = lax.rem(me + 3, N_DEV)
        right = lax.rem(me + 1, N_DEV)
        group = (me, left, right, lax.rem(me + 2, N_DEV))
        odd = lax.rem(me, 2) == 1

        fr = first_rows
        ld_wq0 = pltpu.make_async_copy(wq_hbm.at[pl.ds(0, fr)], wq_f32.at[pl.ds(0, fr)], ld_sem.at[0])
        ld_wq1 = pltpu.make_async_copy(wq_hbm.at[pl.ds(fr, D_MODEL - fr)], wq_f32.at[pl.ds(fr, D_MODEL - fr)], ld_sem.at[1])
        ld_wo = pltpu.make_async_copy(wo_hbm, wo_f32, ld_sem.at[2])
        ld_x = pltpu.make_async_copy(x_hbm, x_f32, ld_sem.at[3])
        ld_k, ld_v = [], []
        for s in range(4):
            rows = pl.ds(pl.multiple_of(group[s] * GRP, GRP), GRP)
            bs = pl.ds(me * B_LOC, B_LOC)
            ld_k.append(pltpu.make_async_copy(kt_hbm.at[bs, rows], k_f32.at[s], ld_sem.at[4 + 2 * s]))
            ld_v.append(pltpu.make_async_copy(vt_hbm.at[bs, rows], v_f32.at[s], ld_sem.at[5 + 2 * s]))
        ld_wq0.start()

        bar = pltpu.get_barrier_semaphore()
        if asym:
            @pl.when(me != 2)
            def _():
                for n in (left, right):
                    pl.semaphore_signal(bar, inc=1, device_id=(n,), device_id_type=MESH)
        else:
            for n in (left, right):
                pl.semaphore_signal(bar, inc=1, device_id=(n,), device_id_type=MESH)

        ld_wq1.start()
        ld_wo.start()
        ld_x.start()
        for s in range(4):
            ld_k[s].start()
            ld_v[s].start()

        def rcopy(src, dst, sem, to):
            return pltpu.make_async_remote_copy(src, dst, send_sem, recv_sem.at[sem], device_id=(to,), device_id_type=MESH)

        to = (right, left)
        slot = (LEFT, RIGHT)

        def wq_first(d, rows):
            return rcopy(wq_all.at[2 * OWN + d, rows], wq_all.at[2 * slot[d] + d, rows], 0 + d, to[d])

        def wq_second(d):
            return rcopy(wq_all.at[2 * OWN + 1 - d], wq_all.at[2 * slot[d] + 1 - d], 2 + d, to[d])

        def wq_fwd(d):
            return rcopy(wq_all.at[2 * slot[d] + d], wq_all.at[2 * DIAG + d], 4 + d, to[d])

        def wo_first(d):
            return rcopy(wo_all.at[2 * OWN + d], wo_all.at[2 * slot[d] + d], 6 + d, to[d])

        def wo_second(d):
            return rcopy(wo_all.at[2 * OWN + 1 - d], wo_all.at[2 * slot[d] + 1 - d], 8 + d, to[d])

        def wo_fwd(d, j):
            return rcopy(wo_all.at[2 * slot[d] + d, j], wo_all.at[2 * DIAG + d, j], 10 + 2 * j + d, to[d])

        r0, r1 = pl.ds(0, fr // 2), pl.ds(fr // 2, (D_MODEL - fr) // 2)

        with scope("wq0"):
            ld_wq0.wait()
            for a in range(2):
                wq_all[a, r0, :] = to_words(wq_f32[0:fr, a * PAIR:(a + 1) * PAIR])

        if asym:
            with scope("bar"):
                @pl.when(odd)
                def _():
                    pl.semaphore_wait(bar, 1)

                @pl.when(jnp.logical_not(odd))
                def _():
                    pl.semaphore_wait(bar, 2)

                @pl.when(me == 2)
                def _():
                    for n in (left, right):
                        pl.semaphore_signal(ready_sem, inc=1, device_id=(n,), device_id_type=MESH)

                @pl.when(me != 1)
                def _():
                    wq_first(0, r0).start()

                @pl.when(me != 3)
                def _():
                    wq_first(1, r0).start()
        else:
            with scope("bar"):
                pl.semaphore_wait(bar, 2)
                for d in range(2):
                    wq_first(d, r0).start()

        with scope("wq1"):
            ld_wq1.wait()
            for a in range(2):
                wq_all[a, r1, :] = to_words(wq_f32[fr:D_MODEL, a * PAIR:(a + 1) * PAIR])

        if asym:
            with scope("bar2"):
                @pl.when(me != 1)
                def _():
                    wq_first(0, r1).start()

                @pl.when(me != 3)
                def _():
                    wq_first(1, r1).start()

                @pl.when(odd)
                def _():
                    pl.semaphore_wait(ready_sem, 1)

                @pl.when(me == 1)
                def _():
                    wq_first(0, r0).start()
                    wq_first(0, r1).start()

                @pl.when(me == 3)
                def _():
                    wq_first(1, r0).start()
                    wq_first(1, r1).start()
        else:
            for d in range(2):
                wq_first(d, r1).start()
        for d in range(2):
            wq_second(d).start()

        with scope("wo_cast"):
            ld_wo.wait()
            for a in range(2):
                for j in range(4):
                    wo_all[a, j] = to_words(wo_f32[a * PAIR:(a + 1) * PAIR, j * 128:(j + 1) * 128])
        with scope("x_cast"):
            ld_x.wait()
            x_bf[...] = to_words(x_f32[...])

        lane = lax.broadcasted_iota(jnp.int32, (BLK, 128), 1)
        lo = lane < BLK
        lo_w = lax.broadcasted_iota(jnp.int32, (32, 128), 1) < DH

        def prep_k(s):
            ld_k[s].wait()
            for a in range(2):
                for t in range(4):
                    b, bp = divmod(t, 2)
                    kt = k_f32[s, b, a * PAIR:(a + 1) * PAIR, bp * 128:(bp + 1) * 128]
                    kk = to_words((kt * SCALE).astype(BF16).T)
                    k0, k1 = kk[0:32], kk[32:64]
                    k_lhs[2 * s + a, t, 0] = jnp.where(lo_w, k0, k1)
                    k_lhs[2 * s + a, t, 1] = jnp.where(lo_w, k1, k0)

        def attend(pieces):
            w = jnp.concatenate([from_words(wq_all[p]) for p in pieces], axis=1)
            qs = [jnp.dot(from_words(x_bf[t * 64:(t + 1) * 64]), w, preferred_element_type=F32) for t in range(4)] if qsplit else None
            if not qsplit:
                q = jnp.dot(from_words(x_bf[...]), w, preferred_element_type=F32)
                qs = [q[t * 128:(t + 1) * 128] for t in range(4)]
            tiles = [(i, p, t) for t in range(4) for i, p in enumerate(pieces)]
            nt = (((1,), (1,)), ((), ()))
            scores = []
            for i, p, t in tiles:
                q0 = qs[t][0:BLK, i * PAIR:(i + 1) * PAIR]
                q1 = qs[t][BLK:128, i * PAIR:(i + 1) * PAIR]
                wa = jnp.concatenate([jnp.where(lo, q0, 0.0), jnp.where(lo, 0.0, q1)], axis=0).astype(BF16)
                wb = jnp.concatenate([jnp.where(lo, 0.0, q0), jnp.where(lo, q1, 0.0)], axis=0).astype(BF16)
                scores.append((lax.dot_general(from_words(k_lhs[p, t, 0]), wa, nt, preferred_element_type=F32),
                               lax.dot_general(from_words(k_lhs[p, t, 1]), wb, nt, preferred_element_type=F32)))
            probs = []
            for sa, sb in scores:
                ea = jnp.exp2(sa - jnp.max(sa, axis=0, keepdims=True))
                eb = jnp.exp2(sb - jnp.max(sb, axis=0, keepdims=True))
                ra = 1.0 / jnp.sum(ea, axis=0, keepdims=True)
                rb = 1.0 / jnp.sum(eb, axis=0, keepdims=True)
                probs.append((ea, eb, ra, rb))
            outs = []
            for (i, p, t), (ea, eb, ra, rb) in zip(tiles, probs):
                s, a = divmod(p, 2)
                b, bp = divmod(t, 2)
                cts = []
                for h, (e0, e1, n0, n1) in enumerate(((ea, eb, ra, rb), (eb, ea, rb, ra))):
                    pw = jnp.concatenate([jnp.where(lo, e0, 0.0), jnp.where(lo, 0.0, e1)], axis=0).astype(BF16)
                    vt = v_f32[s, b, a * PAIR + h * DH:a * PAIR + (h + 1) * DH, bp * 128:(bp + 1) * 128].astype(BF16)
                    cts.append(jnp.dot(vt, pw, preferred_element_type=F32) * jnp.where(lo[0:1], n0, n1))
                outs.append(jnp.concatenate(cts, axis=0))
            for (i, p, t), ct in zip(tiles, outs):
                ctx[p, t * 64:(t + 1) * 64, :] = to_words(ct.astype(BF16).T)

        def oproj(pieces, j, rows=slice(0, TOK // 2)):
            c = jnp.concatenate([from_words(ctx[p, rows]) for p in pieces], axis=1)
            w = jnp.concatenate([from_words(wo_all[p, j]) for p in pieces], axis=0)
            return jnp.dot(c, w, preferred_element_type=F32)

        with scope("own"):
            prep_k(OWN)
            ld_v[OWN].wait()
            attend([0, 1])
        full = pl.ds(0, D_MODEL // 2)
        with scope("w_wq1"):
            for d in range(2):
                wq_first(d, full).wait_recv()
                wq_fwd(d).start()
            for d in range(2):
                wo_first(d).start()
            for d in range(2):
                wo_second(d).start()
        with scope("att1"):
            prep_k(LEFT)
            prep_k(RIGHT)
            ld_v[LEFT].wait()
            ld_v[RIGHT].wait()
            attend([2 * LEFT, 2 * RIGHT + 1])
        with scope("o_own"):
            for j in range(4):
                acc[j] = oproj([0, 1], j)
        with scope("w_wq2"):
            for d in range(2):
                wq_second(d).wait_recv()
        with scope("att2"):
            attend([2 * LEFT + 1, 2 * RIGHT])
            prep_k(DIAG)
            ld_v[DIAG].wait()
        with scope("w_wq3"):
            for d in range(2):
                wq_fwd(d).wait_recv()
        with scope("att3"):
            attend([2 * DIAG, 2 * DIAG + 1])
        with scope("w_wo1"):
            for d in range(2):
                wo_first(d).wait_recv()
            for j in range(4):
                for d in range(2):
                    wo_fwd(d, j).start()
        with scope("o1"):
            for j in range(4):
                acc[j] += oproj([2 * LEFT, 2 * RIGHT + 1], j)
        with scope("w_wo2"):
            for d in range(2):
                wo_second(d).wait_recv()
        with scope("o2"):
            for j in range(4):
                acc[j] += oproj([2 * LEFT + 1, 2 * RIGHT], j)
        for j in range(4):
            with scope(f"w_wo3_{j}"):
                for d in range(2):
                    wo_fwd(d, j).wait_recv()
            with scope(f"o3_{j}"):
                for m in range(2):
                    o = oproj([2 * DIAG, 2 * DIAG + 1], j, slice(m * 128, (m + 1) * 128))
                    out_ref[m * 256:(m + 1) * 256, j * 128:(j + 1) * 128] = (acc[j, m * 256:(m + 1) * 256] + o).astype(out_ref.dtype)
        with scope("w_send"):
            pltpu.make_async_copy(wq_all.at[pl.ds(0, 6)], wq_all.at[pl.ds(0, 6)], send_sem).wait()
            pltpu.make_async_copy(wo_all.at[pl.ds(0, 6)], wo_all.at[pl.ds(0, 6)], send_sem).wait()

    def fn(x, Wq, K_ext, V_ext, Wo):
        nb = K_ext.shape[0]
        kt = jnp.transpose(K_ext, (0, 2, 3, 1)).reshape(nb, N_DEV * GRP, SEQ)
        vt = jnp.transpose(V_ext, (0, 2, 3, 1)).reshape(nb, N_DEV * GRP, SEQ)
        hbm = pl.BlockSpec(memory_space=pltpu.HBM)
        out = pl.pallas_call(
            body,
            out_shape=jax.ShapeDtypeStruct((TOK, D_MODEL), out_dtype),
            in_specs=[hbm] * 5,
            out_specs=pl.BlockSpec(memory_space=pltpu.VMEM),
            scratch_shapes=[
                pltpu.VMEM((TOK, D_MODEL), F32),
                pltpu.VMEM((D_MODEL, GRP), F32),
                pltpu.VMEM((GRP, D_MODEL), F32),
                pltpu.VMEM((4, B_LOC, GRP, SEQ), F32),
                pltpu.VMEM((4, B_LOC, GRP, SEQ), F32),
                pltpu.VMEM((TOK // 2, D_MODEL), U32),
                pltpu.VMEM((8, D_MODEL // 2, PAIR), U32),
                pltpu.VMEM((8, 4, PAIR // 2, 128), U32),
                pltpu.VMEM((8, 4, 2, 32, PAIR), U32),
                pltpu.VMEM((8, TOK // 2, PAIR), U32),
                pltpu.VMEM((4, TOK, 128), F32),
                pltpu.SemaphoreType.DMA((12,)),
                pltpu.SemaphoreType.DMA,
                pltpu.SemaphoreType.DMA((18,)),
                pltpu.SemaphoreType.REGULAR,
            ],
            compiler_params=pltpu.CompilerParams(
                collective_id=0, disable_semaphore_checks=nochk, disable_bounds_checks=nochk,
                vmem_limit_bytes=64 * 1024 * 1024),
        )(x.reshape(TOK, D_MODEL), Wq, kt, vt, Wo)
        return out.reshape(B_LOC, SEQ, D_MODEL)

    return fn


def pallas_dist_sparse_attn_strided_htp_bs_b2_sq256_skv256_hq4_dh64_kernel(x, Wq, K_ext, V_ext, Wo):
    return make()(x, Wq, K_ext, V_ext, Wo)
```

```python
import contextlib

import jax
import jax.numpy as jnp
import numpy as np
from jax import lax
from jax.experimental import pallas as pl
from jax.experimental.pallas import tpu as pltpu

N_DEV = 4
B_LOC = 2
SEQ = 256
D_MODEL = 512
TOK = B_LOC * SEQ
DH = 64
BLK = 64
GRP = 256
PAIR = 128
SCALE = 0.125 * 1.4426950408889634

OWN, LEFT, RIGHT, DIAG = range(4)
MESH = pl.DeviceIdType.MESH
BF16 = jnp.bfloat16
F32 = jnp.float32
I32 = jnp.int32


def _i32(v):
    return int(np.array(v, np.uint32).view(np.int32))


SIGN_MAN = _i32(0x807F807F)
EXPO = 0x7F807F80
TOP = _i32(0x80000000)
BOTH = 0x00010001
STREAM_BITS = 54
SM_ROWS, LOW_ROW, FLAG_ROW, TAIL_ROW, WIRE = 128, 128, 160, 176, 184


def shl(v, n):
    return v << n if n >= 0 else lax.shift_right_logical(v, jnp.full_like(v, -n))


def shr(v, n):
    return lax.shift_right_logical(v, n)


def to_words(v):
    return pltpu.bitcast(v.astype(BF16), I32)


def from_words(w):
    return pltpu.bitcast(w, BF16)


def pack_sign_man(w):
    n = w.shape[0] // 2
    b = w[n:] & SIGN_MAN
    return (w[:n] & SIGN_MAN) | shl(b, 8) | shl(b, -24)


def unpack_sign_man(sm):
    t = sm & EXPO
    return jnp.concatenate([sm & SIGN_MAN, shl(t, -8) | shl(t, 24)], axis=0)


def both(v):
    return v | shl(v, 16)


def partner(v):
    return pltpu.roll(v, 4, 0)


def reverse_bits(v):
    for n, m in ((1, 0x55555555), (2, 0x33333333), (4, 0x0F0F0F0F), (8, 0x00FF00FF)):
        v = (shl(v, -n) & m) | shl(v & m, n)
    return shl(v, -16) | shl(v, 16)


def tree(op, vs):
    while len(vs) > 1:
        vs = [op(vs[i], vs[i + 1]) for i in range(0, len(vs), 2)]
    return vs[0]


def pack_exponents(w):
    ws = [w[8 * j:8 * j + 8] for j in range(32)]
    e = [shl(v, -7) & (0xFF * BOTH) for v in ws]
    as_f32 = lambda v: lax.bitcast_convert_type(v & 0x7F800000, F32)
    top = tree(jnp.maximum, [as_f32(v) for v in ws] + [as_f32(shl(v, 16)) for v in ws])
    top = shl(lax.bitcast_convert_type(jnp.maximum(top, partner(top)), I32), -23)
    base = both(top)
    dist = [base - v for v in e]
    cost = []
    for turn in range(3):
        c = tree(jnp.add, [(d + (8 - turn) * BOTH if turn else d) & (4 * BOTH) for d in dist])
        c = (c & 0xFFFF) + shl(c, -16)
        cost.append(c + partner(c))
    turn = jnp.where(cost[2] < jnp.minimum(cost[0], cost[1]), 2, jnp.where(cost[1] < cost[0], 1, 0))
    back = both(8 - turn)
    low, flag, runs = [None] * 4, [None] * 2, []
    for h in range(2):
        n = jnp.zeros_like(top)
        run = jnp.zeros_like(top)
        for i in range(16):
            j = 16 * h + i
            d = dist[j]
            d = (d & (0xF8 * BOTH)) | ((d + back) & (7 * BOTH))
            r = shl(d & (3 * BOTH), 2 * (j % 8))
            f = shl((d + 0xFC * BOTH) & (0x100 * BOTH), 7 - i)
            low[j // 8] = r if j % 8 == 0 else low[j // 8] | r
            flag[h] = f if i == 0 else flag[h] | f
            for q in (shl(d, -2) & 63, shl(d, -18)):
                n = n + q
                run = run | shr(jnp.full_like(n, TOP), n & 31)
        runs.append((shl(run, 1), n))
    (run0, n0), (run1, n1) = runs
    used = n0 + n1
    lost = jnp.where((n0 > 31) | (n1 > 31) | (used + partner(used) > STREAM_BITS), 1, 0)
    turn = jnp.where(lost + partner(lost) > 0, 3, turn)
    n0 = n0 & 31
    hi = run0 | shr(run1, n0)
    lo = shl(run1, 1) << (31 - n0)
    upper = lax.broadcasted_iota(I32, top.shape, 0) < 4
    head = jnp.where(upper, shl(top, -3), shl(top & 7, 2) | turn)
    tail = shl(head, 27) | ((shl(hi, -5) | reverse_bits(partner(shl(hi, 27) | shl(lo, -5)))) & 0x07FFFFFF)
    return jnp.concatenate(low + flag + [tail], axis=0)


def read_head(tail):
    upper = lax.broadcasted_iota(I32, tail.shape, 0) < 4
    mine, other = shl(tail, -27), shl(partner(tail), -27)
    head = jnp.where(upper, shl(mine, 5) | other, shl(other, 5) | mine)
    return shl(head, -2), head & 3


def unpack_exponents(code):
    tail = code[48:56]
    top, turn = read_head(tail)
    base, turn = shl(both(top), 7), shl(both(turn), 7)
    more = reverse_bits(partner(tail))
    hi, lo = shl(tail, 5) | shl(more, -27), shl(more, 5)
    out = []
    for h in range(2):
        cur = shl(hi, -1) | TOP
        flag = code[32 + 8 * h:40 + 8 * h]
        seen = None
        for i in range(16):
            j = 16 * h + i
            q0 = lax.clz(cur ^ (shl(flag, 16 + i) & TOP))
            cur = cur << q0
            q1 = lax.clz(cur ^ (shl(flag, i) & TOP))
            cur = cur << q1
            q = shl(q0, 9) | shl(q1, 25)
            d = q | (shl(code[8 * (j // 8):8 * (j // 8) + 8], 7 - 2 * (j % 8)) & (0x180 * BOTH))
            out.append(base - ((q & (0x7C00 * BOTH)) | ((d + turn) & (0x380 * BOTH))))
            if h == 0:
                seen = q if i == 0 else seen + q
        if h == 0:
            n0 = (shl(seen, -9) + shl(seen, -25)) & 31
            hi = (hi << n0) | shr(shl(lo, -1), 31 - n0)
    return jnp.concatenate(out, axis=0)


def make(out_dtype=BF16, scopes=False, chunks=(32, 64, 128, 288), early=3, nochk=True, force_slow=False):
    starts = [sum(chunks[:i]) for i in range(len(chunks))]
    NC = len(chunks)

    def scope(name):
        return jax.named_scope(name) if scopes else contextlib.nullcontext()

    def body(x_hbm, wq_hbm, kt_hbm, vt_hbm, wo_hbm, out_ref,
             x_f32, wq_f32, wo_f32, k_f32, v_f32,
             x_bf, plain, wq_wire, wo_wire, k_lhs, ctx, acc,
             ld_sem, send_sem, recv_sem, ready_sem, plain_sem):
        me = lax.axis_index("i")
        left = (me + 3) & 3
        right = (me + 1) & 3
        diag = (me + 2) & 3
        group = (me, left, right, diag)
        odd = (me & 1) == 1

        ld_wq = [pltpu.make_async_copy(wq_hbm.at[pl.ds(s, n)], wq_f32.at[pl.ds(s, n)], ld_sem.at[i])
                 for i, (s, n) in enumerate(zip(starts, chunks))]
        ld_wo = pltpu.make_async_copy(wo_hbm, wo_f32, ld_sem.at[NC])
        ld_x = pltpu.make_async_copy(x_hbm, x_f32, ld_sem.at[NC + 1])
        stage_pieces = ((2 * OWN, 2 * OWN + 1), (2 * LEFT, 2 * RIGHT + 1), (2 * LEFT + 1, 2 * RIGHT), (2 * DIAG, 2 * DIAG + 1))

        def kv_load(hbm, buf, p, sem):
            rows = pl.ds(pl.multiple_of(group[p // 2] * GRP + (p % 2) * PAIR, PAIR), PAIR)
            return pltpu.make_async_copy(hbm.at[pl.ds(me * B_LOC, B_LOC), rows], buf.at[p], ld_sem.at[sem])

        ld_k = [[kv_load(kt_hbm, k_f32, p, NC + 2 + 2 * s) for p in ps] for s, ps in enumerate(stage_pieces)]
        ld_v = [[kv_load(vt_hbm, v_f32, p, NC + 3 + 2 * s) for p in ps] for s, ps in enumerate(stage_pieces)]
        for cp in ld_wq:
            cp.start()

        bar = pltpu.get_barrier_semaphore()

        @pl.when(me != 2)
        def _():
            for n in (left, right):
                pl.semaphore_signal(bar, inc=1, device_id=(n,), device_id_type=MESH)

        ld_wo.start()
        ld_x.start()
        for s in range(4):
            for cp in ld_k[s] + ld_v[s]:
                cp.start()

        @pl.when(odd)
        def _():
            pl.semaphore_wait(bar, 1)

        @pl.when(jnp.logical_not(odd))
        def _():
            pl.semaphore_wait(bar, 2)

        @pl.when(me == 2)
        def _():
            for n in (left, right):
                pl.semaphore_signal(ready_sem, inc=1, device_id=(n,), device_id_type=MESH)

        to = (right, left)
        slot = (LEFT, RIGHT)

        def rcopy(buf, src, dst, rows, sem, d):
            return pltpu.make_async_remote_copy(buf.at[src, rows], buf.at[dst, rows], send_sem, recv_sem.at[sem + d],
                                                device_id=(to[d],), device_id_type=MESH)

        whole = pl.ds(0, WIRE)

        code = pl.ds(SM_ROWS, WIRE - SM_ROWS)

        def wq_first(d, rows=whole):
            return rcopy(wq_wire, 2 * OWN + d, 2 * slot[d] + d, rows, 0, d)

        def wq_second(d, rows=whole):
            return rcopy(wq_wire, 2 * OWN + 1 - d, 2 * slot[d] + 1 - d, rows, 2, d)

        def wq_fwd(d):
            return rcopy(wq_wire, 2 * slot[d] + d, 2 * DIAG + d, whole, 4, d)

        def wo_codes(d):
            return rcopy(wo_wire, pl.ds(2 * OWN, 2), pl.ds(2 * slot[d], 2), code, 6, d)

        def wo_first(d):
            return rcopy(wo_wire, 2 * OWN + d, 2 * slot[d] + d, pl.ds(0, SM_ROWS), 8, d)

        def wo_second(d, part):
            return rcopy(wo_wire, 2 * OWN + 1 - d, 2 * slot[d] + 1 - d, pl.ds(64 * part, 64), 10 + 2 * part, d)

        def wo_fwd(d, j):
            return rcopy(wo_wire, 2 * slot[d] + d, 2 * DIAG + d, code if j < 0 else pl.ds(32 * j, 32), 16 + 2 * j, d)

        def start_known(make_copies):
            for d in range(2):
                @pl.when(me != 1 + 2 * d)
                def _():
                    for cp in make_copies(d):
                        cp.start()

        for i, (s, n) in enumerate(zip(starts, chunks)):
            with scope(f"wq{i}"):
                ld_wq[i].wait()
                w = to_words(wq_f32[s:s + n, :])
                for a in range(2):
                    wa = w[:, a * PAIR:(a + 1) * PAIR]
                    wq_wire[a, s // 4:(s + n) // 4, :] = pack_sign_man(wa)
                    plain[OWN, a, s // 2:(s + n) // 2, :] = wa
                rows = pl.ds(s // 4, n // 4)
                start_known(lambda d: [wq_first(d, rows)] + ([wq_second(d, rows)] if i < early else []))
        sent = sum(chunks[:early]) // 4

        with scope("ready"):
            @pl.when(odd)
            def _():
                pl.semaphore_wait(ready_sem, 1)

            for d in range(2):
                @pl.when(me == 1 + 2 * d)
                def _():
                    wq_first(d, pl.ds(0, SM_ROWS)).start()
                    if sent:
                        wq_second(d, pl.ds(0, sent)).start()

        with scope("wq_exp"):
            for a in range(2):
                wq_wire[a, SM_ROWS:WIRE, :] = pack_exponents(plain[OWN, a])
            for d in range(2):
                wq_first(d, pl.ds(SM_ROWS, WIRE - SM_ROWS)).start()
            for d in range(2):
                wq_second(d, pl.ds(sent, WIRE - sent)).start()

        lo = lax.broadcasted_iota(I32, (BLK, 128), 1) < BLK
        lo_w = lax.broadcasted_iota(I32, (32, 128), 1) < DH

        def prep_k(pieces):
            for p in pieces:
                for t in range(4):
                    b, bp = divmod(t, 2)
                    kt = k_f32[p, b, :, bp * 128:(bp + 1) * 128]
                    kk = to_words((kt * SCALE).astype(BF16).T)
                    k0, k1 = kk[0:32], kk[32:64]
                    k_lhs[p, t, 0] = jnp.where(lo_w, k0, k1)
                    k_lhs[p, t, 1] = jnp.where(lo_w, k1, k0)

        def unpack_wq(p):
            sm = jnp.concatenate([unpack_sign_man(wq_wire[p, s // 4:(s + n) // 4, :]) for s, n in zip(starts, chunks)], axis=0)
            return sm | unpack_exponents(wq_wire[p, SM_ROWS:WIRE, :])

        def unpack_wo(p, j, ex):
            r = 32 * j
            return unpack_sign_man(wo_wire[p, r:r + 32, :]) | ex[64 * j:64 * j + 64]

        def q_proj(ws):
            w = jnp.concatenate([from_words(v) for v in ws], axis=1)
            return jnp.dot(from_words(x_bf[...]), w, preferred_element_type=F32)

        def attend(pieces, q):
            tiles = [(i, p, t) for t in range(4) for i, p in enumerate(pieces)]
            nt = (((1,), (1,)), ((), ()))
            scores = []
            for i, p, t in tiles:
                q0 = q[t * 128:t * 128 + BLK, i * PAIR:(i + 1) * PAIR]
                q1 = q[t * 128 + BLK:(t + 1) * 128, i * PAIR:(i + 1) * PAIR]
                wa = jnp.concatenate([jnp.where(lo, q0, 0.0), jnp.where(lo, 0.0, q1)], axis=0).astype(BF16)
                wb = jnp.concatenate([jnp.where(lo, 0.0, q0), jnp.where(lo, q1, 0.0)], axis=0).astype(BF16)
                scores.append((lax.dot_general(from_words(k_lhs[p, t, 0]), wa, nt, preferred_element_type=F32),
                               lax.dot_general(from_words(k_lhs[p, t, 1]), wb, nt, preferred_element_type=F32)))
            probs = []
            for sa, sb in scores:
                ea = jnp.exp2(sa - jnp.max(sa, axis=0, keepdims=True))
                eb = jnp.exp2(sb - jnp.max(sb, axis=0, keepdims=True))
                ra = 1.0 / jnp.sum(ea, axis=0, keepdims=True)
                rb = 1.0 / jnp.sum(eb, axis=0, keepdims=True)
                probs.append((ea, eb, ra, rb))
            outs = []
            for (i, p, t), (ea, eb, ra, rb) in zip(tiles, probs):
                b, bp = divmod(t, 2)
                cts = []
                for h, (e0, e1, n0, n1) in enumerate(((ea, eb, ra, rb), (eb, ea, rb, ra))):
                    pw = jnp.concatenate([jnp.where(lo, e0, 0.0), jnp.where(lo, 0.0, e1)], axis=0).astype(BF16)
                    vt = v_f32[p, b, h * DH:(h + 1) * DH, bp * 128:(bp + 1) * 128].astype(BF16)
                    cts.append(jnp.dot(vt, pw, preferred_element_type=F32) * jnp.where(lo[0:1], n0, n1))
                outs.append(jnp.concatenate(cts, axis=0))
            for (i, p, t), ct in zip(tiles, outs):
                ctx[p, t * 64:(t + 1) * 64, :] = to_words(ct.astype(BF16).T)

        def o_proj(pieces, ws, rows=slice(0, TOK // 2)):
            c = jnp.concatenate([from_words(ctx[p, rows]) for p in pieces], axis=1)
            w = jnp.concatenate([from_words(v) for v in ws], axis=0)
            return jnp.dot(c, w, preferred_element_type=F32)

        def wait_all(cps):
            for cp in cps:
                cp.wait()

        def wo_exponents(pieces):
            return [unpack_exponents(wo_wire[p, SM_ROWS:WIRE, :]) for p in pieces]

        def o_stage(pieces, ex, js):
            for j in js:
                acc[j] += o_proj(pieces, [unpack_wo(p, j, e) for p, e in zip(pieces, ex)])

        def both_ways(make_copy, *a):
            return [make_copy(d, *a) for d in range(2)]

        def start(cps):
            for cp in cps:
                cp.start()

        def arrived(cps):
            for cp in cps:
                cp.wait_recv()

        with scope("wo_pack"):
            ld_wo.wait()
            w = to_words(wo_f32[...])
            for a in range(2):
                wa = jnp.concatenate([w[a * 64:(a + 1) * 64, j * 128:(j + 1) * 128] for j in range(4)], axis=0)
                plain[OWN, 2 + a] = wa
                for j in range(4):
                    wo_wire[a, 32 * j:32 * j + 32, :] = pack_sign_man(wa[64 * j:64 * j + 64])
                wo_wire[a, SM_ROWS:WIRE, :] = pack_exponents(wa)
            start(both_ways(wo_codes))
        with scope("x_cast"):
            ld_x.wait()
            x_bf[...] = to_words(x_f32[...])
        with scope("B2"):
            q = q_proj([plain[OWN, 0], plain[OWN, 1]])
        with scope("k0"):
            wait_all(ld_k[0])
            prep_k(stage_pieces[0])
        with scope("att0"):
            wait_all(ld_v[0])
            attend(stage_pieces[0], q)
        with scope("w3"):
            arrived(both_ways(wq_first))
            start(both_ways(wq_fwd) + both_ways(wo_first))
            wait_all(ld_k[1])
        with scope("B3"):
            for j in range(4):
                acc[j] = o_proj(stage_pieces[0], [plain[OWN, 2 + a, 64 * j:64 * j + 64] for a in range(2)])
            q = q_proj([unpack_wq(p) for p in stage_pieces[1]])
            prep_k(stage_pieces[1])
        with scope("w4"):
            arrived(both_ways(wq_second))
            wait_all(ld_v[1] + ld_k[2])
        with scope("B4"):
            attend(stage_pieces[1], q)
            q = q_proj([unpack_wq(p) for p in stage_pieces[2]])
            prep_k(stage_pieces[2])
        with scope("w4b"):
            arrived(both_ways(wo_codes))
            start(both_ways(wo_fwd, -1) + both_ways(wo_second, 0) + both_ways(wo_second, 1))
            wait_all(ld_v[2])
        with scope("B4b"):
            attend(stage_pieces[2], q)
            ex1 = wo_exponents(stage_pieces[1])
            ex2 = wo_exponents(stage_pieces[2])
        with scope("w5"):
            arrived(both_ways(wq_fwd))
            wait_all(ld_k[3] + ld_v[3])
        with scope("B5"):
            q = q_proj([unpack_wq(p) for p in stage_pieces[3]])
            prep_k(stage_pieces[3])
        with scope("w6"):
            arrived(both_ways(wo_first))
            for j in range(4):
                start(both_ways(wo_fwd, j))
        with scope("B6"):
            attend(stage_pieces[3], q)
            o_stage(stage_pieces[1], ex1, range(4))
        with scope("w7"):
            arrived(both_ways(wo_fwd, -1) + both_ways(wo_second, 0))
        with scope("B7"):
            o_stage(stage_pieces[2], ex2, (0, 1))
            ex = wo_exponents(stage_pieces[3])
        with scope("w8"):
            arrived(both_ways(wo_second, 1))
        with scope("B8"):
            o_stage(stage_pieces[2], ex2, (2, 3))
            bad = jnp.zeros((8, 128), F32)
            for buf in (wq_wire, wo_wire):
                for p in range(8):
                    bad = jnp.where(read_head(buf[p, TAIL_ROW:WIRE, :])[1] == 3, 1.0, bad)
            unpackable = jnp.max(bad) > 0.0
        for j in range(4):
            with scope(f"w_wo3_{j}"):
                for d in range(2):
                    wo_fwd(d, j).wait_recv()
            with scope(f"o3_{j}"):
                ws = [unpack_wo(p, j, e) for p, e in zip(stage_pieces[3], ex)]
                for m in range(2):
                    o = o_proj(stage_pieces[3], ws, slice(m * 128, (m + 1) * 128))
                    out_ref[m * 256:(m + 1) * 256, j * 128:(j + 1) * 128] = (acc[j, m * 256:(m + 1) * 256] + o).astype(out_ref.dtype)
        with scope("w_send"):
            for buf in (wq_wire, wo_wire):
                v = buf.at[pl.ds(0, 6)]
                pltpu.make_async_copy(v, v, send_sem).wait()

        @pl.when(unpackable | force_slow)
        def _():
            cps = [pltpu.make_async_remote_copy(plain.at[OWN], plain.at[s], plain_sem.at[0], plain_sem.at[s],
                                                device_id=(n,), device_id_type=MESH)
                   for s, n in ((LEFT, right), (RIGHT, left), (DIAG, diag))]
            for cp in cps:
                cp.start()
            for cp in cps:
                cp.wait_recv()
            v = plain.at[pl.ds(1, 3)]
            pltpu.make_async_copy(v, v, plain_sem.at[0]).wait()
            acc[...] = jnp.zeros(acc.shape, F32)

            def step(s, carry):
                pieces = (2 * s, 2 * s + 1)
                attend(pieces, q_proj([plain[s, 0], plain[s, 1]]))
                for j in range(4):
                    acc[j] += o_proj(pieces, [plain[s, 2 + a, 64 * j:64 * j + 64] for a in range(2)])
                return carry

            lax.fori_loop(0, 4, step, 0)
            for j in range(4):
                out_ref[:, j * 128:(j + 1) * 128] = acc[j].astype(out_ref.dtype)

    def fn(x, Wq, K_ext, V_ext, Wo):
        nb = K_ext.shape[0]
        kt = jnp.transpose(K_ext, (0, 2, 3, 1)).reshape(nb, N_DEV * GRP, SEQ)
        vt = jnp.transpose(V_ext, (0, 2, 3, 1)).reshape(nb, N_DEV * GRP, SEQ)
        hbm = pl.BlockSpec(memory_space=pltpu.HBM)
        out = pl.pallas_call(
            body,
            out_shape=jax.ShapeDtypeStruct((TOK, D_MODEL), out_dtype),
            in_specs=[hbm] * 5,
            out_specs=pl.BlockSpec(memory_space=pltpu.VMEM),
            scratch_shapes=[
                pltpu.VMEM((TOK, D_MODEL), F32),
                pltpu.VMEM((D_MODEL, GRP), F32),
                pltpu.VMEM((GRP, D_MODEL), F32),
                pltpu.VMEM((8, B_LOC, PAIR, SEQ), F32),
                pltpu.VMEM((8, B_LOC, PAIR, SEQ), F32),
                pltpu.VMEM((TOK // 2, D_MODEL), I32),
                pltpu.VMEM((4, 4, 256, 128), I32),
                pltpu.VMEM((8, WIRE, 128), I32),
                pltpu.VMEM((8, WIRE, 128), I32),
                pltpu.VMEM((8, 4, 2, 32, PAIR), I32),
                pltpu.VMEM((8, TOK // 2, PAIR), I32),
                pltpu.VMEM((4, TOK, 128), F32),
                pltpu.SemaphoreType.DMA((NC + 10,)),
                pltpu.SemaphoreType.DMA,
                pltpu.SemaphoreType.DMA((24,)),
                pltpu.SemaphoreType.REGULAR,
                pltpu.SemaphoreType.DMA((4,)),
            ],
            compiler_params=pltpu.CompilerParams(
                collective_id=0, disable_semaphore_checks=nochk, disable_bounds_checks=nochk,
                vmem_limit_bytes=64 * 1024 * 1024),
        )(x.reshape(TOK, D_MODEL), Wq, kt, vt, Wo)
        return out.reshape(B_LOC, SEQ, D_MODEL)

    return fn


def pallas_dist_sparse_attn_strided_htp_bs_b2_sq256_skv256_hq4_dh64_kernel(x, Wq, K_ext, V_ext, Wo):
    return make()(x, Wq, K_ext, V_ext, Wo)
```

```python
import jax
import jax.numpy as jnp
from jax import lax
from jax.experimental import pallas as pl
from jax.experimental.pallas import tpu as pltpu

N_DEV = 4
B_LOC = 2
SEQ = 256
D_MODEL = 512
TOK = B_LOC * SEQ
DH = 64
GRP = 256
PAIR = 128
SCALE = 0.125 * 1.4426950408889634

OWN, LEFT, RIGHT, DIAG = range(4)
STAGES = ((2 * OWN, 2 * OWN + 1), (2 * LEFT, 2 * RIGHT + 1), (2 * LEFT + 1, 2 * RIGHT), (2 * DIAG, 2 * DIAG + 1))

CHUNKS = ((0, 32), (32, 64), (96, 128), (224, 256), (480, 32))
EARLY = 3

BF16 = jnp.bfloat16
F32 = jnp.float32
I32 = jnp.int32


SM_ROWS, HEAD_ROW, WIRE_ROWS = 128, 144, 176
STRING_WORDS = 30
HOLD = (5, 5, 5, 5, 4, 4, 4, 4, 3, 3, 3, 3, 2, 2, 2, 1)
MODE_AT = (880, 1250, 1400, 1780, 1920)
DOES_NOT_FIT = 7


def _i32(v):
    return v - (1 << 32) if v >> 31 else v


def _rep(byte):
    return _i32(byte * 0x01010101)


SIGN_MAN = _i32(0x807F807F)
EXPO = 0x7F807F80


def _shr(v, n):
    return lax.shift_right_logical(v, n)


def _shift(v, n):
    if n == 0:
        return v
    return v << n if n > 0 else _shr(v, jnp.full_like(v, -n))


def _to_words(v):
    return pltpu.bitcast(v.astype(BF16), I32)


def _from_words(w):
    return pltpu.bitcast(w, BF16)


def _spread(byte):
    v = byte | _shift(byte, 8)
    return v | _shift(v, 16)


def _tree(op, vs):
    while len(vs) > 1:
        vs = [op(vs[i], vs[i + 1]) for i in range(0, len(vs), 2)]
    return vs[0]


def _all_sublanes(op, v):
    for n in (4, 2, 1):
        v = op(v, pltpu.roll(v, n, 0))
    return v


def _running_sum(v, sub):
    for n in (1, 2, 4):
        v = v + jnp.where(sub >= n, pltpu.roll(v, n, 0), 0)
    return v


def _rotate_first_eight(t, by):
    big = (t + _rep(0x78)) & _rep(0x80)
    u = t + by
    return u ^ ((u ^ t) & ((big - _shift(big, -7)) | _rep(0x78)))


def _swap_zero_two(t, swap):
    return t ^ (swap & ~(_shift(t + _rep(0x7C), -6) | _shift(t, 1)))


def _pack_sign_man(w):
    n = w.shape[0] // 2
    b = w[n:] & SIGN_MAN
    return (w[:n] & SIGN_MAN) | _shift(b, 8) | _shift(b, -24)


def _unpack_sign_man(sm):
    b = sm & EXPO
    return jnp.concatenate([sm & SIGN_MAN, _shift(b, -8) | _shift(b, 24)], axis=0)


def _pack_exponents(w):
    ws = [w[8 * j:8 * j + 8] for j in range(32)]
    sub = lax.broadcasted_iota(I32, ws[0].shape, 0)
    powers = [lax.bitcast_convert_type(v & 0x7F800000, F32) for v in ws + [_shift(v, 16) for v in ws]]
    top = _all_sublanes(jnp.maximum, _tree(jnp.maximum, powers))
    top = _shift(lax.bitcast_convert_type(top, I32), -23)
    base = _spread(top)
    dist = [base - ((_shift(ws[2 * i], -7) & 0x00FF00FF) | (_shift(ws[2 * i + 1], 1) & _i32(0xFF00FF00)))
            for i in range(16)]
    lost = _tree(jnp.bitwise_or, dist) & _rep(0xC0)
    fours = [_tree(jnp.add, dist[i:i + 4]) for i in range(0, 16, 4)]
    total = _tree(jnp.add, [v & 0x00FF00FF for v in fours] + [_shift(v, -8) & 0x00FF00FF for v in fours])
    total = _all_sublanes(jnp.add, (total & 0xFFFF) + _shift(total, -16))
    mode = sum(jnp.where(total > t, 1, 0) for t in MODE_AT)
    back, swap = _spread(8 - _shift(mode, -1)), _spread(_shift(mode & 1, 1))

    one = jnp.ones_like(top)
    low, string, length = [None] * 2, [], None
    for i in reversed(range(16)):
        rank = _swap_zero_two(_rotate_first_eight(dist[i], back), swap)
        bit = _shift(rank & _rep(1), i % 8)
        low[i // 8] = bit if i % 8 == 7 else low[i // 8] | bit
        ends = (_shift(rank, -1) & _rep(0x1F)) + (_rep(1) - 1)
        ends = ends + _shift(ends, 8)
        ends = ends + _shift(ends, 16)
        run = _tree(jnp.bitwise_or, [one << (_shift(ends, -8 * k) & 31) for k in range(4)])
        last = _shift(ends, -24)
        n = last + 1
        lost = lost | (n & -32)
        length = n if i == 15 else length + n
        if i == 0 or HOLD[i - 1] > HOLD[i]:
            lost = lost | jnp.where(length > 32 * HOLD[i], 1, 0)
        up, down = n & 31, ~last & 31
        carry = [run] + [_shr(v, down) for v in string]
        string = [(string[k] << up) | carry[k] if k < len(string) else carry[k] for k in range(HOLD[i])]

    end = _running_sum(length, sub)
    lost = _all_sublanes(jnp.bitwise_or, lost | jnp.where(end > 32 * STRING_WORDS, 1, 0))
    mode = jnp.where(lost != 0, DOES_NOT_FIT, mode)
    start = end - length
    up = start & 31
    carry = [_shr(_shift(v, -1), 31 - up) for v in string]
    words = [string[0] << up] + [(v << up) | c for v, c in zip(string[1:], carry)] + carry[-1:]
    for n in (1, 2, 4, 8, 16):
        move = (start & (32 * n)) != 0
        words = [jnp.where(move, words[k - n] if k >= n else 0, words[k] if k < len(words) else 0)
                 for k in range(min(len(words) + n, STRING_WORDS))]
    head = ((pltpu.roll(length, 1, 0) - 64) & 0x7F) | (_shr(_shift(mode, 8), sub) & 0x80)
    head = jnp.where(sub == 0, top, head) << _shift(sub & 3, 3)
    words = [jnp.where(sub < 4, head, 0), jnp.where(sub < 4, 0, head)] + words
    rows = []
    for v in range(4):
        part = words[8 * v:8 * v + 8]
        for n in (4, 2, 1):
            part = [jnp.where((sub & n) == 0, part[k] | pltpu.roll(part[k], 8 - n, 0),
                              part[k + n] | pltpu.roll(part[k + n], n, 0)) for k in range(n)]
        rows += part
    return jnp.concatenate(low + rows, axis=0)


def _read_mode(head):
    return (_shift(head, -15) & 1) | (_shift(head, -22) & 2) | (_shift(head, -29) & 4)


def _unpack_exponents(rows):
    low = [rows(0, 8), rows(8, 8)]
    sub = lax.broadcasted_iota(I32, low[0].shape, 0)
    words = [jnp.broadcast_to(rows(16 + k, 1), sub.shape) for k in range(2 + STRING_WORDS)]
    mode = _read_mode(words[0])
    base, turn, swap = _spread(words[0] & 0xFF), _spread(_shift(mode, -1)), _spread(_shift(mode & 1, 1))
    before = (_shr(jnp.where(sub < 4, words[0], words[1]), _shift(sub & 3, 3)) & 0x7F) + 64
    start = _running_sum(jnp.where(sub == 0, 0, before), sub)
    words = words[2:]
    for n in (16, 8, 4, 2, 1):
        move = (start & (32 * n)) != 0
        words = [jnp.where(move, words[k + n], words[k]) if k + n < len(words) else words[k]
                 for k in range(HOLD[0] + n)]
    down = start & 31
    string = [_shr(words[k], down) | (_shift(words[k + 1], 1) << (31 - down)) for k in range(HOLD[0])]
    out = []
    for i in range(16):
        rest, ones = string[0], []
        for _ in range(4):
            cleared = rest & (rest - 1)
            ones.append(lax.bitcast_convert_type((rest ^ cleared).astype(F32), I32))
            rest = cleared
        if i < 15:
            last = _shift(ones[3], -23) - 127
            down, up = (last + 1) & 31, ~last & 31
            string = [_shr(string[k], down) | (string[k + 1] << up) if k + 1 < len(string) else _shr(string[k], down)
                      for k in range(HOLD[i + 1])]
        ends = _shift(ones[0], -23) | _shift(ones[1], -15) | _shift(ones[2], -7) | _shift(ones[3], 1)
        rank = _shift(ends - _shift(ends, 8) - (_rep(1) + 126), 1) | (_shift(low[i // 8], -(i % 8)) & _rep(1))
        e = base - _rotate_first_eight(_swap_zero_two(rank, swap), turn)
        out += [_shift(e, 7) & EXPO, _shift(e, -1) & EXPO]
    return jnp.concatenate(out, axis=0)


(WQ_HEAD, WQ_FIRST, WQ_SECOND_CODE, WQ_SECOND, WO_FIRST_CODE, WO_SECOND_CODE, WQ_RELAY_CODE, WQ_RELAY,
 WO_FIRST, WO_RELAY_CODE, WO_SECOND, _, WO_RELAY, _, _, _, PLAIN, PLAIN_RELAY) = range(18)
N_MESSAGES = 18


def _body(x_hbm, wq_hbm, kt_hbm, vt_hbm, wo_hbm, out_ref,
          x_f32, wq_f32, wo_f32, k_f32, v_f32, x_bf, wq_head, plain, wq_wire, wo_wire, k_lhs, ctx, acc,
          load_sem, send_sem, recv_sem, ready_sem):
    me = lax.axis_index("i")
    left, right = (me + 3) & 3, (me + 1) & 3
    owner = (me, left, right, (me + 2) & 3)

    def start(copies):
        for cp in copies:
            cp.start()

    def loaded(copies):
        for cp in copies:
            cp.wait()

    def arrived(copies):
        for cp in copies:
            cp.wait_send()
        for cp in copies:
            cp.wait_recv()

    def signal_neighbours(sem):
        for n in (left, right):
            pl.semaphore_signal(sem, inc=1, device_id=(n,), device_id_type=pl.DeviceIdType.MESH)

    n_chunks = len(CHUNKS)
    ld_wq = [pltpu.make_async_copy(wq_hbm.at[pl.ds(s, n)], wq_f32.at[pl.ds(s, n)], load_sem.at[i])
             for i, (s, n) in enumerate(CHUNKS)]
    ld_wo = pltpu.make_async_copy(wo_hbm, wo_f32, load_sem.at[n_chunks])
    ld_x = pltpu.make_async_copy(x_hbm, x_f32, load_sem.at[n_chunks + 1])

    def kv_load(hbm, buf, p, sem):
        rows = pl.ds(pl.multiple_of(owner[p // 2] * GRP + (p % 2) * PAIR, PAIR), PAIR)
        return pltpu.make_async_copy(hbm.at[pl.ds(me * B_LOC, B_LOC), rows], buf.at[p], load_sem.at[sem])

    ld_k = [[kv_load(kt_hbm, k_f32, p, n_chunks + 2 + p) for p in ps] for ps in STAGES]
    ld_v = [[kv_load(vt_hbm, v_f32, p, n_chunks + 10 + p) for p in ps] for ps in STAGES]

    to, seen_as = (right, left), (LEFT, RIGHT)

    def remote(src, dst, message, d):
        return pltpu.make_async_remote_copy(src, dst, send_sem.at[2 * message + d], recv_sem.at[2 * message + d],
                                            device_id=(to[d],), device_id_type=pl.DeviceIdType.MESH)

    def first(buf, rows, message, ways=(0, 1)):
        return [remote(buf.at[d, rows], buf.at[2 * seen_as[d] + d, rows], message, d) for d in ways]

    def second(buf, rows, message, ways=(0, 1)):
        return [remote(buf.at[1 - d, rows], buf.at[2 * seen_as[d] + 1 - d, rows], message, d) for d in ways]

    def relay(buf, rows, message):
        return [remote(buf.at[2 * seen_as[d] + d, rows], buf.at[2 * DIAG + d, rows], message, d) for d in range(2)]

    sign_man, code = pl.ds(0, SM_ROWS), pl.ds(SM_ROWS, WIRE_ROWS - SM_ROWS)
    head_at, head_rows = CHUNKS[-1]
    head = [remote(wq_hbm.at[pl.ds(head_at, head_rows), pl.ds((1 - d) * PAIR, PAIR)], wq_head.at[d], WQ_HEAD, d)
            for d in range(2)]
    wq_second_code = second(wq_wire, code, WQ_SECOND_CODE)
    wo_codes = first(wo_wire, code, WO_FIRST_CODE) + second(wo_wire, code, WO_SECOND_CODE)
    wq_relay_code, wq_relay = relay(wq_wire, code, WQ_RELAY_CODE), relay(wq_wire, sign_man, WQ_RELAY)
    wo_first, wo_relay_code = first(wo_wire, sign_man, WO_FIRST), relay(wo_wire, code, WO_RELAY_CODE)
    wo_second = [second(wo_wire, pl.ds(64 * h, 64), WO_SECOND + h) for h in range(2)]
    wo_relay = [relay(wo_wire, pl.ds(32 * j, 32), WO_RELAY + j) for j in range(4)]

    barrier = pltpu.get_barrier_semaphore()
    odd = (me & 1) == 1
    ld_wq[0].start()
    for d in range(2):
        @pl.when(to[d] == 0)
        def _():
            pl.semaphore_wait(barrier, 1)
            head[d].start()

    start(ld_wq[1:])
    pl.when(me != 2)(lambda: signal_neighbours(barrier))
    start([ld_wo, ld_x])
    for s in range(4):
        start(ld_k[s] + ld_v[s])

    @pl.when(jnp.logical_not(odd))
    def _():
        pl.semaphore_wait(barrier, 2)
        pl.when(me == 2)(lambda: signal_neighbours(ready_sem))
        start(head)

    for i, (s, n) in enumerate(CHUNKS):
        ld_wq[i].wait()
        w = _to_words(wq_f32[s:s + n, :])
        sm = _pack_sign_man(w)
        for a in range(2):
            wq_wire[a, s // 4:(s + n) // 4, :] = sm[:, a * PAIR:(a + 1) * PAIR]
            plain[OWN, a, s // 2:(s + n) // 2, :] = w[:, a * PAIR:(a + 1) * PAIR]
        rows = pl.ds(s // 4, n // 4)
        for d in range(2):
            @pl.when(to[d] != 2)
            def _():
                start(first(wq_wire, rows, WQ_FIRST, [d]))
                if i < EARLY:
                    start(second(wq_wire, rows, WQ_SECOND, [d]))

    early_rows = CHUNKS[EARLY][0] // 4
    for d in range(2):
        @pl.when(to[d] == 2)
        def _():
            pl.semaphore_wait(ready_sem, 1)
            start(first(wq_wire, sign_man, WQ_FIRST, [d]) + [head[d]]
                  + second(wq_wire, pl.ds(0, early_rows), WQ_SECOND, [d]))

    for a in range(2):
        wq_wire[a, SM_ROWS:WIRE_ROWS, :] = _pack_exponents(plain[OWN, a])
    start(first(wq_wire, code, WQ_FIRST) + wq_second_code
          + second(wq_wire, pl.ds(early_rows, head_at // 4 - early_rows), WQ_SECOND))

    ld_wo.wait()
    w = _to_words(wo_f32[...])
    for a in range(2):
        tiles = [w[64 * a:64 * a + 64, 128 * j:128 * j + 128] for j in range(4)]
        piece = jnp.concatenate(tiles, axis=0)
        plain[OWN, 2 + a] = piece
        wo_wire[a, 0:SM_ROWS, :] = jnp.concatenate([_pack_sign_man(t) for t in tiles], axis=0)
        wo_wire[a, SM_ROWS:WIRE_ROWS, :] = _pack_exponents(piece)
    start(wo_codes)

    lo = lax.broadcasted_iota(I32, (DH, 128), 1) < DH
    lo_words = lax.broadcasted_iota(I32, (DH // 2, 128), 1) < DH

    def plain_pair(shard, at, rows=slice(None)):
        return [plain[shard, at + a, rows] for a in range(2)]

    def exponents(buf, pieces):
        return [_unpack_exponents(lambda at, n: buf[p, SM_ROWS + at:SM_ROWS + at + n, :]) for p in pieces]

    def wq_words(pieces, expo, chunks=CHUNKS):
        return [jnp.concatenate([_unpack_sign_man(wq_wire[p, s // 4:(s + n) // 4, :]) | e[s // 2:(s + n) // 2]
                                 for s, n in chunks], axis=0) for p, e in zip(pieces, expo)]

    def wo_words(pieces, expo, j):
        return [_unpack_sign_man(wo_wire[p, 32 * j:32 * j + 32, :]) | e[64 * j:64 * j + 64]
                for p, e in zip(pieces, expo)]

    def q_proj(words):
        w = jnp.concatenate([_from_words(v) for v in words], axis=1)
        return jnp.dot(_from_words(x_bf[...]), w, preferred_element_type=F32)

    def prepare_k(pieces):
        for p in pieces:
            for t in range(4):
                kt = k_f32[p, t // 2, :, (t % 2) * 128:(t % 2 + 1) * 128]
                k = _to_words((kt * SCALE).astype(BF16).T)
                k_lhs[p, t, 0] = jnp.where(lo_words, k[:32], k[32:])
                k_lhs[p, t, 1] = jnp.where(lo_words, k[32:], k[:32])

    def diagonal(a, b):
        return jnp.concatenate([jnp.where(lo, a, 0.0), jnp.where(lo, 0.0, b)], axis=0).astype(BF16)

    def attend(pieces, q):
        tiles = [(i, p, t) for t in range(4) for i, p in enumerate(pieces)]
        nt = (((1,), (1,)), ((), ()))
        scores = []
        for i, p, t in tiles:
            q0 = q[t * 128:t * 128 + DH, i * PAIR:(i + 1) * PAIR]
            q1 = q[t * 128 + DH:(t + 1) * 128, i * PAIR:(i + 1) * PAIR]
            crossed = jnp.concatenate([jnp.where(lo, 0.0, q0), jnp.where(lo, q1, 0.0)], axis=0).astype(BF16)
            scores.append([lax.dot_general(_from_words(k_lhs[p, t, c]), rhs, nt, preferred_element_type=F32)
                           for c, rhs in enumerate((diagonal(q0, q1), crossed))])
        weights = []
        for pair in scores:
            e = [jnp.exp2(s - jnp.max(s, axis=0, keepdims=True)) for s in pair]
            weights.append((e, [1.0 / jnp.sum(v, axis=0, keepdims=True) for v in e]))
        outs = []
        for (i, p, t), (e, inv) in zip(tiles, weights):
            heads = []
            for h in range(2):
                vt = v_f32[p, t // 2, h * DH:(h + 1) * DH, (t % 2) * 128:(t % 2 + 1) * 128].astype(BF16)
                heads.append(jnp.dot(vt, diagonal(e[h], e[1 - h]), preferred_element_type=F32)
                             * jnp.where(lo[0:1], inv[h], inv[1 - h]))
            outs.append(jnp.concatenate(heads, axis=0))
        for (i, p, t), ct in zip(tiles, outs):
            ctx[p, t * 64:(t + 1) * 64, :] = _to_words(ct.astype(BF16).T)

    def o_proj(pieces, words, rows=slice(None)):
        c = jnp.concatenate([_from_words(ctx[p, rows]) for p in pieces], axis=1)
        w = jnp.concatenate([_from_words(v) for v in words], axis=0)
        return jnp.dot(c, w, preferred_element_type=F32)

    ld_x.wait()
    x_bf[...] = _to_words(x_f32[...])
    q0 = q_proj(plain_pair(OWN, 0))
    loaded(ld_k[0])
    prepare_k(STAGES[0])

    arrived(first(wq_wire, pl.ds(0, WIRE_ROWS), WQ_FIRST))
    start(wq_relay_code + wq_relay + wo_first)
    loaded(ld_v[0])
    attend(STAGES[0], q0)

    loaded(ld_k[1])
    for j in range(4):
        acc[j] = o_proj(STAGES[0], plain_pair(OWN, 2, slice(64 * j, 64 * j + 64)))
    expo = exponents(wq_wire, STAGES[1])

    arrived(wq_second_code)
    q1 = q_proj(wq_words(STAGES[1], expo))
    prepare_k(STAGES[1])
    expo = exponents(wq_wire, STAGES[2])

    arrived(second(wq_wire, pl.ds(0, head_at // 4), WQ_SECOND) + head + wo_codes)
    start(wo_relay_code + wo_second[0] + wo_second[1])
    loaded(ld_k[2])
    q2 = q_proj([jnp.concatenate([v, _to_words(wq_head[d])], axis=0)
                 for d, v in enumerate(wq_words(STAGES[2], expo, CHUNKS[:-1]))])
    prepare_k(STAGES[2])
    expo1 = exponents(wo_wire, STAGES[1])

    arrived(wq_relay_code)
    loaded(ld_v[1] + ld_v[2])
    attend(STAGES[1], q1)
    attend(STAGES[2], q2)
    expo = exponents(wq_wire, STAGES[3])

    arrived(wq_relay)
    loaded(ld_k[3] + ld_v[3])
    q3 = q_proj(wq_words(STAGES[3], expo))
    prepare_k(STAGES[3])
    expo2 = exponents(wo_wire, STAGES[2])

    arrived(wo_first)
    for j in range(4):
        start(wo_relay[j])
    attend(STAGES[3], q3)
    for j in range(4):
        acc[j] += o_proj(STAGES[1], wo_words(STAGES[1], expo1, j))

    arrived(wo_relay_code + wo_second[0])
    for j in (0, 1):
        acc[j] += o_proj(STAGES[2], wo_words(STAGES[2], expo2, j))
    expo = exponents(wo_wire, STAGES[3])

    arrived(wo_second[1])
    for j in (2, 3):
        acc[j] += o_proj(STAGES[2], wo_words(STAGES[2], expo2, j))
    misfit = jnp.zeros((1, 128), F32)
    for buf in (wq_wire, wo_wire):
        for p in range(8):
            misfit = jnp.where(_read_mode(buf[p, HEAD_ROW:HEAD_ROW + 1, :]) == DOES_NOT_FIT, 1.0, misfit)
    incomplete = jnp.max(misfit) > 0.0

    for j in range(4):
        arrived(wo_relay[j])
        words = wo_words(STAGES[3], expo, j)
        for m in range(2):
            rows = slice(m * 256, (m + 1) * 256)
            o = acc[j, rows] + o_proj(STAGES[3], words, slice(m * 128, (m + 1) * 128))
            out_ref[rows, j * 128:(j + 1) * 128] = o.astype(out_ref.dtype)

    @pl.when(incomplete)
    def _():
        direct = [remote(plain.at[OWN], plain.at[seen_as[d]], PLAIN, d) for d in range(2)]
        start(direct)
        arrived(direct)
        relayed = [remote(plain.at[seen_as[d], pl.ds(2 * d, 2)], plain.at[DIAG, pl.ds(2 * d, 2)], PLAIN_RELAY, d)
                   for d in range(2)]
        start(relayed)
        arrived(relayed)
        acc[...] = jnp.zeros(acc.shape, F32)

        def add_shard(s, carry):
            pieces = (2 * s, 2 * s + 1)
            attend(pieces, q_proj(plain_pair(s, 0)))
            for j in range(4):
                acc[j] += o_proj(pieces, plain_pair(s, 2, slice(64 * j, 64 * j + 64)))
            return carry

        lax.fori_loop(0, N_DEV, add_shard, 0)
        for j in range(4):
            out_ref[:, j * 128:(j + 1) * 128] = acc[j].astype(out_ref.dtype)


def pallas_dist_sparse_attn_strided_htp_bs_b2_sq256_skv256_hq4_dh64_kernel(
    x: jax.Array,
    Wq: jax.Array,
    K_ext: jax.Array,
    V_ext: jax.Array,
    Wo: jax.Array,
):
    kt = jnp.transpose(K_ext, (0, 2, 3, 1)).reshape(N_DEV * B_LOC, N_DEV * GRP, SEQ)
    vt = jnp.transpose(V_ext, (0, 2, 3, 1)).reshape(N_DEV * B_LOC, N_DEV * GRP, SEQ)
    out = pl.pallas_call(
        _body,
        out_shape=jax.ShapeDtypeStruct((TOK, D_MODEL), BF16),
        in_specs=[pl.BlockSpec(memory_space=pltpu.HBM)] * 5,
        out_specs=pl.BlockSpec(memory_space=pltpu.VMEM),
        scratch_shapes=[
            pltpu.VMEM((TOK, D_MODEL), F32),
            pltpu.VMEM((D_MODEL, GRP), F32),
            pltpu.VMEM((GRP, D_MODEL), F32),
            pltpu.VMEM((8, B_LOC, PAIR, SEQ), F32),
            pltpu.VMEM((8, B_LOC, PAIR, SEQ), F32),
            pltpu.VMEM((TOK // 2, D_MODEL), I32),
            pltpu.VMEM((2, CHUNKS[-1][1], PAIR), F32),
            pltpu.VMEM((N_DEV, 4, 256, 128), I32),
            pltpu.VMEM((8, WIRE_ROWS, 128), I32),
            pltpu.VMEM((8, WIRE_ROWS, 128), I32),
            pltpu.VMEM((8, 4, 2, DH // 2, PAIR), I32),
            pltpu.VMEM((8, TOK // 2, PAIR), I32),
            pltpu.VMEM((4, TOK, 128), F32),
            pltpu.SemaphoreType.DMA((len(CHUNKS) + 18,)),
            pltpu.SemaphoreType.DMA((2 * N_MESSAGES,)),
            pltpu.SemaphoreType.DMA((2 * N_MESSAGES,)),
            pltpu.SemaphoreType.REGULAR,
        ],
        compiler_params=pltpu.CompilerParams(
            collective_id=0,
            disable_semaphore_checks=True,
            vmem_limit_bytes=64 * 1024 * 1024,
        ),
    )(x.reshape(TOK, D_MODEL), Wq, kt, vt, Wo)
    return out.reshape(B_LOC, SEQ, D_MODEL)
```
